```python
import numpy as np

kernel_name = "dist_ar_xy_y_m256_n256"

def setup_inputs():
    return {"x": np.random.randn(512, 256).astype(np.float32)}

def reference(x: np.ndarray) -> np.ndarray:
    return x.reshape(2, 256, 256).sum(axis=0)
```

```python
import jax
import jax.numpy as jnp
from jax import lax
from jax.experimental import pallas as pl
from jax.experimental.pallas import tpu as pltpu


def pallas_dist_ar_xy_y_m256_n256_kernel(x: jax.Array):
    m, n = x.shape

    def body(x_ref, out_ref, send_buf, recv_buf, send_sem, recv_sem):
        my_x = lax.axis_index("x")
        my_y = lax.axis_index("y")
        nbr = (my_x, 1 - my_y)

        barrier_sem = pltpu.get_barrier_semaphore()
        pl.semaphore_signal(barrier_sem, inc=1, device_id=nbr,
                            device_id_type=pl.DeviceIdType.MESH)
        send_buf[...] = x_ref[...].astype(jnp.bfloat16)
        pl.semaphore_wait(barrier_sem, 1)

        rdma = pltpu.make_async_remote_copy(
            src_ref=send_buf, dst_ref=recv_buf,
            send_sem=send_sem, recv_sem=recv_sem,
            device_id=nbr, device_id_type=pl.DeviceIdType.MESH,
        )
        rdma.start()
        rdma.wait()
        out_ref[...] = x_ref[...] + recv_buf[...].astype(jnp.float32)

    return pl.pallas_call(
        body,
        out_shape=jax.ShapeDtypeStruct((m, n), jnp.float32),
        in_specs=[pl.BlockSpec(memory_space=pltpu.VMEM)],
        out_specs=pl.BlockSpec(memory_space=pltpu.VMEM),
        scratch_shapes=[
            pltpu.VMEM((m, n), jnp.bfloat16),
            pltpu.VMEM((m, n), jnp.bfloat16),
            pltpu.SemaphoreType.DMA,
            pltpu.SemaphoreType.DMA,
        ],
        compiler_params=pltpu.CompilerParams(collective_id=0),
    )(x)
```

```python
import jax
import jax.numpy as jnp
from jax import lax
from jax.experimental import pallas as pl
from jax.experimental.pallas import tpu as pltpu

MESH = pl.DeviceIdType.MESH

NF = (12, 12)
LEAD = ((0, 5, 9, 12, 17, 20, 23, 30), (31, 38, 40, 45, 48, 53, 58, 59))
FC = (2, 1)
BULK = (32, 96, 128)
TAIL = 2
SCRIPT = (("SBBB", "SWPGGPGPGGBBB"), ("SBBB", "GGGGGGBSWPPBB"))


def _rect(t, k=1):
    if k == 1:
        return (pl.ds(8 * (t // 2), 8), pl.ds(128 * (t % 2), 128))
    assert t % 2 == 0 and k % 2 == 0
    return (pl.ds(8 * (t // 2), 8 * (k // 2)), pl.ds(0, 256))


def _plan(nt):
    lead = LEAD[0] + LEAD[1]
    nat = [[t for t in list(range(s * nt // 2, nt)) + list(range(s * nt // 2)) if t not in lead]
           for s in range(2)]
    fwd = [list(LEAD[s]) + nat[s][:NF[s] - len(LEAD[s])] for s in range(2)]
    order, chunks = [], []
    for s in range(2):
        order.append(fwd[s] + [t for t in nat[s] if t not in fwd[0] + fwd[1]])
        assert sorted(order[s] + fwd[1 - s]) == list(range(nt))
        ch, j, tot = [], 0, len(order[s])
        while j < tot:
            rem = tot - j
            if j < len(LEAD[s]) or j % 2 or rem == 1:
                k = 1
            elif j < NF[s]:
                k = min(FC[s], NF[s] - j)
            elif rem <= 5:
                k = 2
            elif rem <= 13:
                k = rem - 4 - rem % 2
            else:
                k = min(10, rem - 12 - rem % 2)
            ch.append((j, k))
            j += k
        chunks.append(ch)
    return order, chunks


def pallas_dist_ar_xy_y_m256_n256_kernel(x: jax.Array):
    m, n = x.shape
    assert n == 256 and sum(BULK) == m
    order, chs = _plan((m // 8) * (n // 128))
    nfc = [sum(1 for j, _ in chs[s] if j < NF[s]) for s in range(2)]
    npmax = max(sc.count("P") for r in SCRIPT for sc in r)
    ngmax = max(sc.count("G") for r in SCRIPT for sc in r)
    nyc = max(len(c) for c in chs)

    def body(x_hbm, out_ref, xv, gbuf, sbuf, rbuf, fbuf, pbuf,
             ld_sems, ys_sems, yr_sems, xs_sems, xr_sems, xrdy):
        my_x = lax.axis_index("x")
        my_y = lax.axis_index("y")
        barrier_sem = pltpu.get_barrier_semaphore()

        def program(s, sy):
            o = 1 - s
            od, ch = order[s], chs[s]
            script = SCRIPT[s][sy]
            npf = script.count("P")
            npr = SCRIPT[s][1 - sy].count("P")
            ynbr = (s, 1 - sy)
            xnbr = (o, sy)

            gl = list(range(npf, npf + script.count("G")))
            bulk, a = [], s * (m // 2)
            for z in BULK:
                bulk.append((a % m, a % m + z))
                a += z
            gloads = [pltpu.make_async_copy(x_hbm.at[_rect(od[j])], gbuf.at[j - npf], ld_sems.at[j - npf])
                      for j in gl]
            bloads = [pltpu.make_async_copy(x_hbm.at[pl.ds(a, b - a)], xv.at[pl.ds(a, b - a)],
                                            ld_sems.at[len(gl) + i])
                      for i, (a, b) in enumerate(bulk)]
            loads = gloads + bloads

            def ycopy(c, src, dst):
                return pltpu.make_async_remote_copy(
                    src_ref=src, dst_ref=dst, send_sem=ys_sems.at[c], recv_sem=yr_sems.at[c],
                    device_id=ynbr, device_id_type=MESH)

            def xcopy(c, j, k):
                return pltpu.make_async_remote_copy(
                    src_ref=rbuf.at[_rect(j, k)], dst_ref=fbuf.at[_rect(j, k)],
                    send_sem=xs_sems.at[c], recv_sem=xr_sems.at[c],
                    device_id=xnbr, device_id_type=MESH)

            ys = []
            gi = bi = 0
            for tok in script:
                if tok == "S":
                    pl.semaphore_signal(barrier_sem, inc=1, device_id=ynbr, device_id_type=MESH)
                    if s == 0:
                        pl.semaphore_signal(barrier_sem, inc=1, device_id=xnbr, device_id_type=MESH)
                elif tok == "W":
                    pl.semaphore_wait(barrier_sem, 1 + s)
                elif tok == "P":
                    c = len(ys)
                    ys.append(ycopy(c, x_hbm.at[_rect(od[c])], pbuf.at[c]))
                    ys[-1].start()
                elif tok == "G":
                    gloads[gi].start()
                    gi += 1
                else:
                    bloads[bi].start()
                    bi += 1
            late_barrier = "W" not in script

            waited = set()

            def wait_load(i):
                if i not in waited:
                    loads[i].wait()
                    waited.add(i)

            def src_tile(j):
                if j in gl:
                    wait_load(j - npf)
                    return gbuf[j - npf]
                r = 8 * (od[j] // 2)
                for i, (a, b) in enumerate(bulk):
                    if a <= r < b:
                        wait_load(len(gl) + i)
                return xv[_rect(od[j])]

            def cast(j, k):
                if k == 1:
                    sbuf[_rect(j)] = src_tile(j).astype(jnp.bfloat16)
                else:
                    for q in range(j, j + k, 2):
                        pair = jnp.concatenate([src_tile(q), src_tile(q + 1)], axis=1)
                        sbuf[_rect(q, 2)] = pair.astype(jnp.bfloat16)

            if late_barrier:
                for j, k in ch:
                    cast(j, k)
                pl.semaphore_wait(barrier_sem, 1 + s)
            for c in range(npf, len(ch)):
                j, k = ch[c]
                if not late_barrier:
                    cast(j, k)
                ys.append(ycopy(c, sbuf.at[_rect(j, k)], rbuf.at[_rect(j, k)]))
                ys[-1].start()
                if c == npf and s == 1:
                    pl.semaphore_signal(xrdy, inc=1, device_id=xnbr, device_id_type=MESH)
            for i in range(len(loads)):
                wait_load(i)

            def yrecv(c):
                j, k = ch[c]
                if c < npr:
                    ycopy(c, pbuf.at[c], pbuf.at[c]).wait_recv()
                else:
                    ycopy(c, sbuf.at[_rect(j, k)], rbuf.at[_rect(j, k)]).wait_recv()

            if s == 0:
                pl.semaphore_wait(xrdy, 1)
            xs = [xcopy(c, *ch[c]) for c in range(nfc[s])]
            for c in range(nfc[s]):
                yrecv(c)
                if c < npr:
                    rbuf[_rect(c)] = pbuf[c].astype(jnp.bfloat16)
                xs[c].start()

            def add(buf, tiles, j, k):
                if k == 1:
                    out_ref[_rect(tiles[j])] = xv[_rect(tiles[j])] + buf[_rect(j)].astype(jnp.float32)
                else:
                    for q in range(j, j + k, 2):
                        v = buf[_rect(q, 2)].astype(jnp.float32)
                        out_ref[_rect(tiles[q])] = xv[_rect(tiles[q])] + v[:, :128]
                        out_ref[_rect(tiles[q + 1])] = xv[_rect(tiles[q + 1])] + v[:, 128:]

            for c in range(nfc[s]):
                if c < npr:
                    out_ref[_rect(od[c])] = xv[_rect(od[c])] + pbuf[c]
                else:
                    add(rbuf, od, *ch[c])

            def ystep(c):
                yrecv(c)
                add(rbuf, od, *ch[c])

            def xstep(c):
                xcopy(c, *chs[o][c]).wait_recv()
                add(fbuf, order[o], *chs[o][c])

            ny, nx = len(ch), nfc[o]
            for c in range(nfc[s], ny - TAIL - 1):
                ystep(c)
            for cp in ys + xs:
                cp.wait_send()
            ystep(ny - TAIL - 1)
            for c in range(nx - TAIL):
                xstep(c)
            for t in range(TAIL):
                ystep(ny - TAIL + t)
                xstep(nx - TAIL + t)

        for s, sy in ((0, 0), (0, 1), (1, 0), (1, 1)):
            pl.when(jnp.logical_and(my_x == s, my_y == sy))(lambda s=s, sy=sy: program(s, sy))

    return pl.pallas_call(
        body,
        out_shape=jax.ShapeDtypeStruct((m, n), jnp.float32),
        in_specs=[pl.BlockSpec(memory_space=pl.ANY)],
        out_specs=pl.BlockSpec(memory_space=pltpu.VMEM),
        scratch_shapes=[
            pltpu.VMEM((m, n), jnp.float32),
            pltpu.VMEM((ngmax, 8, 128), jnp.float32),
            pltpu.VMEM((m, n), jnp.bfloat16),
            pltpu.VMEM((m, n), jnp.bfloat16),
            pltpu.VMEM((8 * ((max(NF) + 3) // 4 * 2), n), jnp.bfloat16),
            pltpu.VMEM((npmax, 8, 128), jnp.float32),
            pltpu.SemaphoreType.DMA((ngmax + len(BULK),)),
            pltpu.SemaphoreType.DMA((nyc,)),
            pltpu.SemaphoreType.DMA((nyc,)),
            pltpu.SemaphoreType.DMA((max(nfc),)),
            pltpu.SemaphoreType.DMA((max(nfc),)),
            pltpu.SemaphoreType.REGULAR,
        ],
        compiler_params=pltpu.CompilerParams(
            collective_id=0, disable_semaphore_checks=True, disable_bounds_checks=True),
    )(x)
```

```python
import jax
import jax.numpy as jnp
from jax import lax
from jax.experimental import pallas as pl
from jax.experimental.pallas import tpu as pltpu

MESH = pl.DeviceIdType.MESH
NT = 64

LEAD = (
    [(14, 22, 0), (7, 15, 0), (12, 20, 1), (9, 17, 1), (30, 38, 1), (2, 3, 1), (28, 36, 0), (25, 33, 0),
     10, 11, 18, 19, 6, 24],
    [(5, 0, 0), (56, 61, 1), (42, 43, 1), (50, 51, 1), (40, 48, 0), (45, 53, 0), (23, 31, 1), (58, 59, 0),
     (40, 48, 1), (45, 53, 1), (58, 59, 1), (23, 31, 0), 32],
)
NFWD = ((12, 12), (12, 13))
BULK = (32, 96, 128)
SCRIPT = (("SBBB", "SWPaPPbcdefghijkBBB"), ("SBBB", "abcdefghijkSWHHHH|BBB"))
SEND_WAIT = 8


def _rect(j, k=1, h=None):
    if h is not None:
        return (pl.ds(8 * (j // 2) + 4 * h, 4), pl.ds(128 * (j % 2), 128))
    if k == 1:
        return (pl.ds(8 * (j // 2), 8), pl.ds(128 * (j % 2), 128))
    assert j % 2 == 0 and k % 2 == 0
    return (pl.ds(8 * (j // 2), 8 * (k // 2)), pl.ds(0, 256))


def _tail_chunks(j, total, first=()):
    ch, first = [], list(first)
    while j < total:
        rem = total - j
        if j % 2 or rem == 1:
            k = 1
        elif first:
            k = first.pop(0)
        elif rem <= 5:
            k = 2
        elif rem <= 13:
            k = rem - 4 - rem % 2
        else:
            k = min(10, rem - 12 - rem % 2)
        ch.append((j, k, None))
        j += k
    return ch


def _f32_chunks(script):
    ch, halves = [], 0
    for tok in script:
        if tok == "P":
            ch.append((halves // 2, 1, None))
            halves += 2
        elif tok == "H":
            ch.append((halves // 2, 1, halves % 2))
            halves += 1
    return ch


def _f32_slots(script):
    return script.count("P") + script.count("H") // 2


def _n_lead(script):
    return sum(tok.islower() for tok in script)


def _plan():
    is_pair = lambda d: isinstance(d, tuple)
    nat = [list(range(s * NT // 2, NT)) + list(range(s * NT // 2)) for s in range(2)]
    order, chunks = [[], []], [[], []]
    for s in range(2):
        order[0].append([t for t in nat[s] if t not in nat[1 - s][:NFWD[0][1 - s]]])
        chunks[0].append([(j, 2, None) for j in range(0, NFWD[0][s], 2)]
                         + _tail_chunks(NFWD[0][s], len(order[0][s])))
    lead = LEAD[0] + LEAD[1]
    pairs = [d for d in lead if is_pair(d)]
    other = [(a, b, 1 - p) for a, b, p in pairs if (a, b, 1 - p) not in pairs]
    other += [t for t in range(NT) if t not in lead and not any(t in d[:2] for d in pairs)]
    for s in range(2):
        ready = lambda d: max(nat[s].index(t) for t in (d[:2] if is_pair(d) else (d,)))
        rest = sorted(LEAD[1 - s][NFWD[1][1 - s]:] + other, key=ready)
        last = [d for d in rest if not is_pair(d)][-8:]
        order[1].append(LEAD[s] + [d for d in rest if d not in last] + last)
        ch, nf32 = _f32_chunks(SCRIPT[s][1]), _f32_slots(SCRIPT[s][1])
        for j in range(nf32, len(LEAD[s])):
            ch += [(j, 1, 0), (j, 1, 1)] if (j == nf32 or s == 1) else [(j, 1, None)]
        chunks[1].append(ch + _tail_chunks(len(LEAD[s]), len(order[1][s]), (4, 6)))
    return order, chunks


def pallas_dist_ar_xy_y_m256_n256_kernel(x: jax.Array):
    m, n = x.shape
    assert (m, n) == (256, 256)
    order, chunks = _plan()
    nfc = [[sum(c[0] < NFWD[y][s] for c in chunks[y][s]) for s in range(2)] for y in range(2)]
    scripts = [sc for r in SCRIPT for sc in r]
    npmax = max(_f32_slots(sc) for sc in scripts)
    ncmax = max(len(_f32_chunks(sc)) for sc in scripts)
    ngmax = max(_n_lead(sc) for sc in scripts)
    nyc = max(len(c) for r in chunks for c in r)
    nxc = max(c for r in nfc for c in r)
    bf16, f32, u32 = jnp.bfloat16, jnp.float32, jnp.uint32

    def body(x_hbm, v_hbm, out_ref, xv, gbuf, tbuf, sbuf, rbuf, fbuf, pbuf, cbuf,
             ld_sems, ys_sems, yr_sems, xs_sems, xr_sems, rdy):
        my_x = lax.axis_index("x")
        my_y = lax.axis_index("y")
        barrier_sem = pltpu.get_barrier_semaphore()

        def hbm_rows(d, h=None):
            a, b, p = d
            if h is not None:
                return v_hbm.at[d[h] // 8, d[h] % 8, :, p]
            if b == a + 1:
                return v_hbm.at[a // 8, pl.ds(a % 8, 2), :, p]
            assert b == a + 8
            return v_hbm.at[pl.ds(a // 8, 2), a % 8, :, p]

        def program(s, sy):
            o = 1 - s
            od, ch = order[sy][s], chunks[sy][s]
            rod, rch, nf = order[1 - sy][s], chunks[1 - sy][s], nfc[1 - sy][s]
            fod, fch, nx = order[1 - sy][o], chunks[1 - sy][o], nfc[1 - sy][o]
            script = SCRIPT[s][sy]
            npf, npr = _f32_slots(script), _f32_slots(SCRIPT[s][1 - sy])
            ncf, ncr = len(_f32_chunks(script)), len(_f32_chunks(SCRIPT[s][1 - sy]))
            ng = _n_lead(script)
            ynbr, xnbr = (s, 1 - sy), (o, sy)
            hub = (s, sy) == (1, 0)

            def lead_load(i):
                d = od[npf + i]
                if i == 0:
                    return [pltpu.make_async_copy(hbm_rows(d, h), gbuf.at[i, h], ld_sems.at[h]) for h in range(2)]
                if isinstance(d, tuple):
                    return [pltpu.make_async_copy(hbm_rows(d), gbuf.at[i], ld_sems.at[i + 1])]
                return [pltpu.make_async_copy(x_hbm.at[_rect(d)], tbuf.at[i], ld_sems.at[i + 1])]

            bulk, r0 = [], s * (m // 2)
            for z in BULK:
                bulk.append((r0 % m, z))
                r0 += z
            loads = [lead_load(i) for i in range(ng)]
            loads += [[pltpu.make_async_copy(x_hbm.at[pl.ds(r, z)], xv.at[pl.ds(r, z)], ld_sems.at[ngmax + 1 + i])]
                      for i, (r, z) in enumerate(bulk)]

            def pwin(j, k, h):
                return pbuf.at[j] if h is None else pbuf.at[j, h]

            def ycopy(c, src, dst):
                return pltpu.make_async_remote_copy(
                    src_ref=src, dst_ref=dst, send_sem=ys_sems.at[c], recv_sem=yr_sems.at[c],
                    device_id=ynbr, device_id_type=MESH)

            def xcopy(c, src, dst):
                return pltpu.make_async_remote_copy(
                    src_ref=src, dst_ref=dst, send_sem=xs_sems.at[c], recv_sem=xr_sems.at[c],
                    device_id=xnbr, device_id_type=MESH)

            ys, nbulk = [], [0]

            def run(tokens):
                for tok in tokens:
                    if tok == "S":
                        pl.semaphore_signal(barrier_sem, inc=1, device_id=ynbr, device_id_type=MESH)
                    elif tok == "W":
                        pl.semaphore_wait(barrier_sem, 1)
                    elif tok in "PH":
                        j, _, h = ch[len(ys)]
                        ys.append(ycopy(len(ys), hbm_rows(od[j], h), pwin(j, 1, h)))
                        ys[-1].start()
                    elif tok == "B":
                        loads[ng + nbulk[0]][0].start()
                        nbulk[0] += 1
                    else:
                        for cp in loads[ord(tok) - ord("a")]:
                            cp.start()

            parts = script.split("|")
            run(parts[0])

            waited, done = set(), set()

            def wait_load(i):
                if i not in waited:
                    loads[i][0].wait()
                    waited.add(i)

            def tile(t):
                for i, (r, z) in enumerate(bulk):
                    if r <= 8 * (t // 2) < r + z:
                        wait_load(ng + i)
                return xv[_rect(t)]

            def slot(j):
                d, i = od[j], j - npf
                if i < ng:
                    wait_load(i)
                    if isinstance(d, tuple):
                        return jnp.concatenate([gbuf[i, 0], gbuf[i, 1]], axis=0)
                    return tbuf[i]
                if not isinstance(d, tuple):
                    return tile(d)
                w = pltpu.bitcast(jnp.concatenate([tile(d[0]), tile(d[1])], axis=0).astype(bf16), u32)
                return pltpu.bitcast((w & jnp.uint32(0xFFFF0000)) if d[2] else (w << 16), f32)

            def cast(j, k, h):
                if ng and j == npf:
                    loads[0][h].wait()
                    waited.add(0)
                    sbuf[_rect(j, 1, h)] = gbuf[0, h].astype(bf16)
                    return
                for q in range(j, j + k):
                    if q not in done:
                        sbuf[_rect(q)] = slot(q).astype(bf16)
                        done.add(q)

            if sy == 0:
                for c in ch:
                    cast(*c)
                pl.semaphore_wait(barrier_sem, 2 if hub else 1)
                if not hub:
                    pl.semaphore_signal(barrier_sem, inc=1, device_id=xnbr, device_id_type=MESH)
            for c in range(ncf, len(ch)):
                cast(*ch[c])
                ys.append(ycopy(c, sbuf.at[_rect(*ch[c])], rbuf.at[_rect(*ch[c])]))
                ys[-1].start()
                if c == ncf:
                    run(parts[1:] and parts[1])
                    if hub:
                        for dst in ((0, 1), (0, 0), (1, 1)):
                            pl.semaphore_signal(rdy, inc=1, device_id=dst, device_id_type=MESH)
            for i in range(len(loads)):
                wait_load(i)

            def yrecv(c):
                dst = pwin(*rch[c]) if c < ncr else rbuf.at[_rect(*rch[c])]
                ycopy(c, dst, dst).wait_recv()

            def xrecv(c):
                dst = fbuf.at[_rect(*fch[c])]
                xcopy(c, dst, dst).wait_recv()

            def pval(j):
                return jnp.concatenate([pbuf[j, 0], pbuf[j, 1]], axis=0)

            if not hub:
                pl.semaphore_wait(rdy, 1)
            xs = []
            for c in range(nf):
                j, _, h = rch[c]
                yrecv(c)
                src = rbuf.at[_rect(*rch[c])]
                if c < ncr:
                    src = cbuf.at[c, pl.ds(0, 8 if h is None else 4)]
                    src[...] = (pval(j) if h is None else pbuf[j, h]).astype(bf16)
                xs.append(xcopy(c, src, fbuf.at[_rect(*rch[c])]))
                xs[-1].start()

            have = {}

            def bits(buf, j):
                v = pval(j).astype(bf16) if (buf is rbuf and j < npr) else buf[_rect(j)]
                return pltpu.bitcast(v.astype(f32), u32)

            def reduce(buf, slots, j, k, h):
                if h == 0:
                    return
                for q in range(j, j + k):
                    d = slots[q]
                    if not isinstance(d, tuple):
                        out_ref[_rect(d)] = xv[_rect(d)] + buf[_rect(q)].astype(f32)
                        continue
                    have[d] = (buf, q)
                    if (d[0], d[1], 1 - d[2]) in have:
                        w = (bits(*have[d[:2] + (0,)]) >> 16) | bits(*have[d[:2] + (1,)])
                        w = pltpu.bitcast(w, bf16).astype(f32)
                        out_ref[_rect(d[0])] = xv[_rect(d[0])] + w[:8]
                        out_ref[_rect(d[1])] = xv[_rect(d[1])] + w[8:]

            for c in range(nf):
                reduce(rbuf, rod, *rch[c])

            def left(chl):
                size = [k if h is None else 0.5 for _, k, h in chl]
                return [sum(size[i + 1:]) for i in range(len(chl))]

            ly, lx = left(rch), left(fch[:nx])
            events = [(-ly[c], "y", c) for c in range(nf, len(rch) - 1)]
            events += [(0.1 - lx[c], "x", c) for c in range(nx - 1)]
            events += [(0.05 - SEND_WAIT, "s", 0)]
            for _, kind, c in sorted(events):
                if kind == "y":
                    yrecv(c)
                    reduce(rbuf, rod, *rch[c])
                elif kind == "x":
                    xrecv(c)
                    reduce(fbuf, fod, *fch[c])
                else:
                    for cp in ys + xs:
                        cp.wait_send()
            yrecv(len(rch) - 1)
            xrecv(nx - 1)
            reduce(rbuf, rod, *rch[-1])
            reduce(fbuf, fod, *fch[nx - 1])

        for s, sy in ((0, 1), (1, 1), (1, 0), (0, 0)):
            pl.when(jnp.logical_and(my_x == s, my_y == sy))(lambda s=s, sy=sy: program(s, sy))

    v = x.reshape(8, 4, 4, 2, 2, 128).transpose(0, 1, 4, 2, 3, 5).reshape(8, 8, 4, 2, 128)
    return pl.pallas_call(
        body,
        out_shape=jax.ShapeDtypeStruct((m, n), jnp.float32),
        in_specs=[pl.BlockSpec(memory_space=pl.ANY)] * 2,
        out_specs=pl.BlockSpec(memory_space=pltpu.VMEM),
        scratch_shapes=[
            pltpu.VMEM((m, n), jnp.float32),
            pltpu.VMEM((ngmax, 2, 4, 128), jnp.float32),
            pltpu.VMEM((ngmax, 8, 128), jnp.float32),
            pltpu.VMEM((m, n), jnp.bfloat16),
            pltpu.VMEM((m, n), jnp.bfloat16),
            pltpu.VMEM((64, n), jnp.bfloat16),
            pltpu.VMEM((npmax, 2, 4, 128), jnp.float32),
            pltpu.VMEM((ncmax, 16, 128), jnp.bfloat16),
            pltpu.SemaphoreType.DMA((ngmax + 1 + len(BULK),)),
            pltpu.SemaphoreType.DMA((nyc,)),
            pltpu.SemaphoreType.DMA((nyc,)),
            pltpu.SemaphoreType.DMA((nxc,)),
            pltpu.SemaphoreType.DMA((nxc,)),
            pltpu.SemaphoreType.REGULAR,
        ],
        compiler_params=pltpu.CompilerParams(
            collective_id=0, disable_semaphore_checks=True),
    )(x, v)
```
